```python
import numpy as np

kernel_name = "dist_matmul_relu_kshard_i_m1024_n1024_k512"

def setup_inputs():
    A = np.random.randn(1024, 2048).astype(np.float32)
    B = np.random.randn(2048, 1024).astype(np.float32)
    return {"A": A, "B": B}

def reference(A: np.ndarray, B: np.ndarray) -> np.ndarray:
    z = A @ B
    return np.maximum(z, 0.0)
```

```python
import jax
import jax.numpy as jnp
from jax import lax
from jax.experimental import pallas as pl
from jax.experimental.pallas import tpu as pltpu

M, N, K = 1024, 1024, 512
Q = M // 4
H = N // 2
XOR = (1, 3)

BF16 = jnp.bfloat16
F32 = jnp.float32

P0_COLS = ((0, 128), (128, 256), (256, 512))
S_ROWS = ((0, 128), (128, 256))
G_ROWS = ((0, 128), (128, 224), (224, 256))


def _body(a_hbm, b_hbm, o_hbm,
          a32, b32, abf, bbf, psend, precv, ssend, srecv, fsend, frecv, grecv,
          acc, ostage, lsem, osem, ssem, rsem):
    k = lax.axis_index("i")
    nbr = tuple(k ^ x for x in XOR)

    def rows_of(r, lo=0, hi=Q):
        return pl.ds(pl.multiple_of((k ^ r) * Q + lo, 8), hi - lo)

    barrier = pltpu.get_barrier_semaphore()
    for l in range(2):
        pl.semaphore_signal(barrier, 1, device_id=(nbr[l],),
                            device_id_type=pl.DeviceIdType.MESH)

    n_load = [0]

    def load(src, dst):
        cp = pltpu.make_async_copy(src, dst, lsem.at[n_load[0]])
        n_load[0] += 1
        cp.start()
        return cp

    la = {2: load(a_hbm.at[rows_of(2)], a32.at[2])}
    lb = {}
    for lo, hi in P0_COLS:
        for h in range(2):
            cols = pl.ds(h * H + lo, hi - lo)
            lb[h, lo] = load(b_hbm.at[:, cols], b32.at[:, cols])
    for r in (1, 3, 0):
        la[r] = load(a_hbm.at[rows_of(r)], a32.at[r])

    n_rc = [0]
    sends = []

    def remote(l, src, dst):
        i = n_rc[0]
        n_rc[0] += 1
        return pltpu.make_async_remote_copy(
            src, dst, ssem.at[i], rsem.at[i], device_id=(nbr[l],),
            device_id_type=pl.DeviceIdType.MESH)

    def send(l, src, dst):
        cp = remote(l, src, dst)
        cp.start()
        sends.append(cp)
        return cp

    n_st = [0]
    stores = []

    def store(r, lo, hi, h=None):
        cols = pl.ds(0, N) if h is None else pl.ds(h * H, H)
        cp = pltpu.make_async_copy(ostage.at[r, pl.ds(lo, hi - lo), cols],
                                   o_hbm.at[rows_of(r, lo, hi), cols],
                                   osem.at[n_st[0]])
        n_st[0] += 1
        cp.start()
        stores.append(cp)

    def mm(r, c0, c1, lo=0, hi=Q):
        return jnp.dot(abf[r, lo:hi, :], bbf[:, c0:c1], preferred_element_type=F32)

    la[2].wait()
    abf[2] = a32[2].astype(BF16)
    p0 = []
    for i, (lo, hi) in enumerate(P0_COLS):
        for h in range(2):
            c0, c1 = h * H + lo, h * H + hi
            lb[h, lo].wait()
            bbf[:, c0:c1] = b32[:, c0:c1].astype(BF16)
            psend[h, 0, :, lo:hi] = mm(2, c0, c1).astype(BF16)
            if i == 0 and h == 0:
                pl.semaphore_wait(barrier, 2)
            cols = pl.ds(lo, hi - lo)
            p0.append(send(h, psend.at[h, 0, :, cols], precv.at[h, 0, :, cols]))

    p1 = []
    for l in range(2):
        r = XOR[l]
        la[r].wait()
        abf[r] = a32[r].astype(BF16)
        psend[l, 1] = mm(r, l * H, (l + 1) * H).astype(BF16)
        p1.append(send(l, psend.at[l, 1], precv.at[l, 1]))

    la[0].wait()
    abf[0] = a32[0].astype(BF16)
    acc[...] = mm(0, 0, N)

    for cp in p0:
        cp.wait_recv()
    s = {}
    for lo, hi in S_ROWS:
        for l in range(2):
            h = 1 - l
            part = mm(XOR[l], h * H, (h + 1) * H, lo, hi)
            ssend[l, lo:hi] = (part + precv[h, 0, lo:hi].astype(F32)).astype(BF16)
            rows = pl.ds(lo, hi - lo)
            s[l, lo] = send(l, ssend.at[l, rows], srecv.at[l, rows])

    for h in range(2):
        p1[h].wait_recv()
        acc[:, h * H:(h + 1) * H] += precv[h, 1].astype(F32)

    f = {}
    for lo, hi in S_ROWS:
        rows = pl.ds(lo, hi - lo)
        for l in range(2):
            h = 1 - l
            s[l, lo].wait_recv()
            z = acc[lo:hi, h * H:(h + 1) * H] + srecv[l, lo:hi].astype(F32)
            fsend[h, lo:hi] = jnp.maximum(z, 0.0).astype(BF16)
        for l in range(2):
            f[l, lo] = send(l, fsend.at[:, rows], frecv.at[l, :, rows])
        for h in range(2):
            ostage[0, lo:hi, h * H:(h + 1) * H] = fsend[h, lo:hi].astype(F32)
        store(0, lo, hi)

    g = {}
    for lo, hi in S_ROWS:
        for l in range(2):
            f[l, lo].wait_recv()
        for glo, ghi in G_ROWS:
            if lo <= glo < hi:
                rows = pl.ds(glo, ghi - glo)
                for l in range(2):
                    g[l, glo] = send(l, frecv.at[1 - l, l, rows], grecv.at[l, rows])
        for l in range(2):
            for h in range(2):
                ostage[XOR[l], lo:hi, h * H:(h + 1) * H] = frecv[l, h, lo:hi].astype(F32)
            store(XOR[l], lo, hi)

    for glo, ghi in G_ROWS:
        for l in range(2):
            g[l, glo].wait_recv()
            ostage[2, glo:ghi, l * H:(l + 1) * H] = grecv[l, glo:ghi].astype(F32)
        store(2, glo, ghi)

    for cp in sends:
        cp.wait_send()
    for cp in stores:
        cp.wait()


def pallas_dist_matmul_relu_kshard_i_m1024_n1024_k512_kernel(A, B):
    n_remote = 2 * (len(P0_COLS) + 1 + 2 * len(S_ROWS) + len(G_ROWS))
    n_load = 4 + 2 * len(P0_COLS)
    n_store = 3 * len(S_ROWS) + len(G_ROWS)
    hbm = pl.BlockSpec(memory_space=pltpu.HBM)
    return pl.pallas_call(
        _body,
        out_shape=jax.ShapeDtypeStruct((M, N), F32),
        in_specs=[hbm, hbm],
        out_specs=hbm,
        scratch_shapes=[
            pltpu.VMEM((4, Q, K), F32),
            pltpu.VMEM((K, N), F32),
            pltpu.VMEM((4, Q, K), BF16),
            pltpu.VMEM((K, N), BF16),
            pltpu.VMEM((2, 2, Q, H), BF16),
            pltpu.VMEM((2, 2, Q, H), BF16),
            pltpu.VMEM((2, Q, H), BF16),
            pltpu.VMEM((2, Q, H), BF16),
            pltpu.VMEM((2, Q, H), BF16),
            pltpu.VMEM((2, 2, Q, H), BF16),
            pltpu.VMEM((2, Q, H), BF16),
            pltpu.VMEM((Q, N), F32),
            pltpu.VMEM((4, Q, N), F32),
            pltpu.SemaphoreType.DMA((n_load,)),
            pltpu.SemaphoreType.DMA((n_store,)),
            pltpu.SemaphoreType.DMA((n_remote,)),
            pltpu.SemaphoreType.DMA((n_remote,)),
        ],
        compiler_params=pltpu.CompilerParams(
            collective_id=0, vmem_limit_bytes=64 * 1024 * 1024),
    )(A, B)
```

```python
import contextlib
import numpy as np
import jax
import jax.numpy as jnp
from jax import lax
from jax.experimental import pallas as pl
from jax.experimental.pallas import tpu as pltpu

M, N, K = 1024, 1024, 512
Q = M // 4
H = Q // 2
XOR = (1, 3)

BF16, F32, U32 = jnp.bfloat16, jnp.float32, jnp.uint32
LOW, SIGN = np.uint32(0x7FFF7FFF), np.uint32(0x80008000)
scope = lambda n: contextlib.nullcontext()

B_COLS = ((0, 128), (128, 256), (256, 384), (384, 512), (512, 768), (768, 1024))
E = 64
NC, GC, GR = 4, 256, 120
PH = NC * GR
WP = 80
WG = 48
N_SEM = 58


def _body(a_hbm, b_hbm, o_ref, a32, b32, abf, bbf, p0s, p0r, p1s, p1r, ss, sr,
          pk, acc, lsem, ssem, rsem):
    k = lax.axis_index("i")
    nbr = tuple(k ^ x for x in XOR)

    def rows_of(r, lo=0, hi=Q):
        return pl.ds(pl.multiple_of((k ^ r) * Q + lo, 16), hi - lo)

    counters = dict(load=0, send=0, recv=0)

    def fresh(kind):
        counters[kind] += 1
        return counters[kind] - 1

    def load(src, dst):
        cp = pltpu.make_async_copy(src, dst, lsem.at[fresh("load")])
        cp.start()
        return cp

    def load_a(slot, r, lo, hi):
        return load(a_hbm.at[rows_of(r, lo, hi)], a32.at[slot, pl.ds(lo, hi - lo)])

    def load_b(c0, c1):
        cols = pl.ds(c0, c1 - c0)
        return load(b_hbm.at[:, cols], b32.at[:, cols])

    lb = [load_b(*B_COLS[0])]
    la_mid = load_a(2, 2, H - E, H + E)

    barrier = pltpu.get_barrier_semaphore()
    for l in range(2):
        pl.semaphore_signal(barrier, 1, device_id=(nbr[l],),
                            device_id_type=pl.DeviceIdType.MESH)

    lb.append(load_b(*B_COLS[1]))
    la_rest = [load_a(2, 2, 0, H - E), load_a(2, 2, H + E, Q)]
    for c in B_COLS[2:]:
        lb.append(load_b(*c))
    la_p1 = [load_a(1, XOR[h], h * H, (h + 1) * H) for h in range(2)]
    la_s = [load_a(3, XOR[1 - h], h * H, (h + 1) * H) for h in range(2)]
    la_own = load_a(0, 0, 0, Q)

    drains = []

    def remote(dev, src, dst, s, r):
        return pltpu.make_async_remote_copy(
            src, dst, ssem.at[s], rsem.at[r], device_id=(dev,),
            device_id_type=pl.DeviceIdType.MESH)

    def send(dev, src, dst, r=None, cond=None):
        s = fresh("send")
        r = fresh("recv") if r is None else r
        if cond is None:
            cp = remote(dev, src, dst, s, r)
            cp.start()
            drains.append(cp.wait_send)
            return cp
        pl.when(cond)(lambda: remote(dev, src, dst, s, r).start())
        drains.append(
            lambda: pl.when(cond)(lambda: remote(dev, src, dst, s, r).wait_send()))

    def arrived(dst, r):
        pltpu.make_async_copy(dst, dst, rsem.at[r]).wait()

    def mm(r, lo, hi, c0, c1):
        return jnp.dot(abf[r, lo:hi, :], bbf[0, :, c0:c1], preferred_element_type=F32)

    def cast_a(r, lo, hi):
        abf[r, lo:hi] = a32[r, lo:hi].astype(BF16)

    def cast_b(c0, c1):
        bbf[0, :, c0:c1] = b32[:, c0:c1].astype(BF16)

    def tile(ref, lo, hi, c0, c1):
        return ref.at[0, pl.ds(lo, hi - lo), pl.ds(c0, c1 - c0)]

    def digit_is(v):
        return k == v

    p0 = []
    wp_r = [fresh("recv") for _ in range(4)]
    for i, (c0, c1) in enumerate(B_COLS):
        with scope(f"wB{i}"):
            lb[i].wait()
        cast_b(c0, c1)
        if i == 0:
            with scope("wAmid"):
                la_mid.wait()
            cast_a(2, H - E, H + E)
        if i < 2:
            p0s[0, H - E:H + E, c0:c1] = mm(2, H - E, H + E, c0, c1).astype(BF16)
            if i == 0:
                with scope("bar"):
                    pl.semaphore_wait(barrier, 2)
            for l, (lo, hi) in enumerate(((H - E, H), (H, H + E))):
                p0.append(send(nbr[l], tile(p0s, lo, hi, c0, c1), tile(p0r, lo, hi, c0, c1)))
        if i == 1:
            for l, (lo, hi) in enumerate(((0, H - E), (H + E, Q))):
                with scope(f"wArest{l}"):
                    la_rest[l].wait()
                cast_a(2, lo, hi)
                p0s[0, lo:hi, 0:c1] = mm(2, lo, hi, 0, c1).astype(BF16)
                p0.append(send(nbr[l], tile(p0s, lo, hi, 0, c1), tile(p0r, lo, hi, 0, c1)))
        if i >= 2:
            p0s[0, :, c0:c1] = mm(2, 0, Q, c0, c1).astype(BF16)
            w = WP if c1 == N else 0
            for l in range(2):
                lo, hi = l * H + w, (l + 1) * H
                p0.append(send(nbr[l], tile(p0s, lo, hi, c0, c1), tile(p0r, lo, hi, c0, c1)))
            for l in range(2 if w else 0):
                turn = k == XOR[l]
                row = pl.multiple_of(jnp.where(turn, Q + l * w, l * H), 16)
                send(jnp.where(turn, nbr[1 - l], nbr[l]),
                     tile(p0s, l * H, l * H + w, c0, c1),
                     p0r.at[0, pl.ds(row, w), pl.ds(c0, c1 - c0)],
                     r=jnp.where(turn, wp_r[2 + l], wp_r[l]))

    with scope("wA1"):
        for cp in la_p1:
            cp.wait()
    cast_a(1, 0, Q)
    p1 = {}
    for c in range(NC):
        c0, c1 = c * GC, (c + 1) * GC
        p1s[0, :, c0:c1] = mm(1, 0, Q, c0, c1).astype(BF16)
        w = WP if c1 == N else 0
        for l in range(2):
            lo, hi = l * H + w, (l + 1) * H
            p1[l, c] = [send(nbr[l], tile(p1s, lo, hi, c0, c1), tile(p1r, lo, hi, c0, c1))]

    for cp in la_s:
        cp.wait()
    cast_a(3, 0, Q)
    la_own.wait()
    cast_a(0, 0, Q)
    acc[...] = mm(0, 0, Q, 0, N)

    for i, cp in enumerate(p0):
        with scope(f"wP0_{i}"):
            cp.wait_recv()
    if WP:
        with scope("wW"):
            @pl.when(k != 0)
            def _():
                for l in range(2):
                    arrived(tile(p0r, l * H, l * H + WP, N - GC, N), wp_r[l])

            @pl.when(k == 2)
            def _():
                for l in range(2):
                    arrived(tile(p0r, Q + l * WP, Q + (l + 1) * WP, N - GC, N), wp_r[2 + l])

    s = {}
    for c in range(NC):
        c0, c1 = c * GC, (c + 1) * GC
        w = WP if c1 == N else 0
        part = mm(3, 0, Q, c0, c1)
        for h in range(2):
            lo, hi = h * H, (h + 1) * H
            if w:
                got = jnp.where(k != 0, p0r[0, lo:lo + w, c0:c1].astype(F32), 0.0)
                ss[0, lo:lo + w, c0:c1] = (part[lo:lo + w] + got).astype(BF16)
            got = p0r[0, lo + w:hi, c0:c1].astype(F32)
            ss[0, lo + w:hi, c0:c1] = (part[lo + w:hi] + got).astype(BF16)
        for l in range(2):
            lo, hi = (1 - l) * H, (2 - l) * H
            s[l, c] = send(nbr[l], tile(ss, lo, hi, c0, c1), tile(sr, lo, hi, c0, c1))
        for l in range(2 if w else 0):
            lo = l * H
            got = jnp.where(k == 2, p0r[0, Q + l * w:Q + (l + 1) * w, c0:c1].astype(F32), 0.0)
            p1s[0, lo:lo + w, c0:c1] = (mm(1, lo, lo + w, c0, c1) + got).astype(BF16)
            p1[l, c].append(send(nbr[l], tile(p1s, lo, lo + w, c0, c1), tile(p1r, lo, lo + w, c0, c1)))

    def out_tile(r, h, c, j):
        lo = h * H + 16 * (j % 8)
        return o_ref.at[rows_of(r, lo, lo + 16), pl.ds(c * GC + 128 * (j // 8), 128)]

    def pack(h, c, z):
        w = pltpu.bitcast(jnp.maximum(z, 0.0).astype(BF16), U32) & LOW
        word = lambda j: w[8 * (j % 8):8 * (j % 8) + 8, 128 * (j // 8):128 * (j // 8) + 128]
        g0 = h * PH + c * GR
        for j in range(15):
            pk[0, g0 + 8 * j:g0 + 8 * j + 8] = word(j) | ((word(15) << (15 - j)) & SIGN)
        o_ref[rows_of(0, h * H, (h + 1) * H), c * GC:(c + 1) * GC] = pltpu.bitcast(w, BF16)

    def unpack(r, h, c):
        g0 = h * PH + c * GR
        last = None
        for j in range(15):
            p = pk[r, g0 + 8 * j:g0 + 8 * j + 8]
            out_tile(r, h, c, j)[...] = pltpu.bitcast(p & LOW, BF16)
            bit = (p & SIGN) >> (15 - j)
            last = bit if last is None else last | bit
        out_tile(r, h, c, 15)[...] = pltpu.bitcast(last, BF16)

    def packed(r, lo, hi):
        return pk.at[r, pl.ds(lo, hi - lo)]

    swing = ((PH - WG, PH), (PH, PH + WG))
    f1 = {}
    for c in range(NC):
        c0, c1 = c * GC, (c + 1) * GC
        for l in range(2):
            h = 1 - l
            with scope(f"wS{l}_{c0}"):
                for cp in p1[h, c]:
                    cp.wait_recv()
                s[l, c].wait_recv()
            lo, hi = h * H, (h + 1) * H
            pack(h, c, acc[lo:hi, c0:c1] + p1r[0, lo:hi, c0:c1].astype(F32)
                 + sr[0, lo:hi, c0:c1].astype(F32))
            g0 = h * PH + c * GR
            f1[l, c] = send(nbr[l], packed(0, g0, g0 + GR), packed(XOR[l], g0, g0 + GR))
    f2w, f2 = [], []
    for l in range(2):
        if WG:
            f2w.append(send(nbr[l], packed(0, *swing[l]), packed(XOR[l], *swing[l])))
        rest = ((0, PH - WG), (PH + WG, 2 * PH))[l]
        f2.append(send(nbr[l], packed(0, *rest), packed(XOR[l], *rest)))

    for c in range(NC):
        for l in range(2):
            with scope(f"wF{l}_{c}"):
                f1[l, c].wait_recv()
    wg_r = [fresh("recv") for _ in range(2)]
    with scope("wF2w"):
        for cp in f2w:
            cp.wait_recv()
    for l in range(2 if WG else 0):
        r = XOR[1 - l]
        send(nbr[l], packed(r, *swing[l]), packed(2, *swing[l]), r=wg_r[l], cond=k != 2)
        send(nbr[l], packed(r, *swing[1 - l]), packed(2, *swing[1 - l]), r=wg_r[1 - l], cond=k == 0)
    early = list(drains)
    del drains[:]
    g = {}
    for c in range(NC):
        for l in range(2):
            lo, hi = l * PH + c * GR, l * PH + (c + 1) * GR
            lo, hi = (lo, min(hi, PH - WG)) if l == 0 else (max(lo, PH + WG), hi)
            g[l, c] = send(nbr[l], packed(XOR[1 - l], lo, hi), packed(2, lo, hi))
    for l in range(2):
        for c in range(NC):
            unpack(XOR[l], 1 - l, c)
    for l in range(2):
        with scope(f"wF2_{l}"):
            f2[l].wait_recv()
        for c in range(NC):
            unpack(XOR[l], l, c)
    with scope("drain0"):
        for drain in early:
            drain()
    with scope("wGw"):
        for h in range(2 if WG else 0):
            arrived(packed(2, *swing[h]), wg_r[h])
    for c in range(NC):
        if c == NC - 1:
            with scope("drain1"):
                for drain in drains[:-2]:
                    drain()
        for l in range(2):
            with scope(f"wG{l}_{c}"):
                g[l, c].wait_recv()
            unpack(2, l, c)
    with scope("drain2"):
        for drain in drains[-2:]:
            drain()
    assert max(counters.values()) <= N_SEM, counters


def pallas_dist_matmul_relu_kshard_i_m1024_n1024_k512_kernel(A, B):
    hbm = pl.BlockSpec(memory_space=pltpu.HBM)
    blk = pltpu.VMEM((1, Q, N), BF16)
    out = pl.pallas_call(
        _body,
        out_shape=pltpu.VMEM((M, N), BF16),
        in_specs=[hbm, hbm],
        out_specs=pl.BlockSpec(memory_space=pltpu.VMEM),
        scratch_shapes=[
            pltpu.VMEM((4, Q, K), F32),
            pltpu.VMEM((K, N), F32),
            pltpu.VMEM((4, Q, K), BF16),
            pltpu.VMEM((1, K, N), BF16),
            blk, pltpu.VMEM((1, Q + 2 * WP, N), BF16), blk, blk, blk, blk,
            pltpu.VMEM((4, 2 * PH, 128), U32),
            pltpu.VMEM((Q, N), F32),
            pltpu.SemaphoreType.DMA((8 + len(B_COLS),)),
            pltpu.SemaphoreType.DMA((N_SEM,)),
            pltpu.SemaphoreType.DMA((N_SEM,)),
        ],
        compiler_params=pltpu.CompilerParams(
            collective_id=0, vmem_limit_bytes=32 * 1024 * 1024,
            disable_semaphore_checks=True),
    )(A, B)
    return out
```

```python
import jax
import jax.numpy as jnp
import numpy as np
from jax import lax
from jax.experimental import pallas as pl
from jax.experimental.pallas import tpu as pltpu

M, N, K = 1024, 1024, 512
Q = M // 4
H = Q // 2
XOR = (1, 3)

BF16, F32, U32 = jnp.bfloat16, jnp.float32, jnp.uint32
LOW, SIGN = np.uint32(0x7FFF7FFF), np.uint32(0x80008000)

B_COLS = ((0, 128), (128, 256), (256, 384), (384, 512), (512, 768), (768, 1024))
E = 64
NC, GC = 4, 256
GR = 120
PH = NC * GR
WP = 80
WG = 48
N_LOADS, N_SENDS, N_RECVS = 14, 60, 60

A_DIAG, A_NEAR, A_SUM, A_OWN = range(4)


def _body(a_hbm, b_hbm, o_ref, a32, b32, p0s, p0r, p1s, p1r, ss, sr, pk, acc,
          lsem, ssem, rsem):
    k = lax.axis_index("i")
    nbr = tuple(k ^ x for x in XOR)

    def rows_of(r, lo, hi):
        return pl.ds(pl.multiple_of((k ^ r) * Q + lo, 16), hi - lo)

    used = dict(load=0, send=0, recv=0)

    def fresh(kind):
        used[kind] += 1
        return used[kind] - 1

    def load(src, dst):
        cp = pltpu.make_async_copy(src, dst, lsem.at[fresh("load")])
        cp.start()
        return cp

    def load_a(slot, r, lo, hi):
        return load(a_hbm.at[rows_of(r, lo, hi)], a32.at[slot, pl.ds(lo, hi - lo)])

    def load_b(c0, c1):
        cols = pl.ds(c0, c1 - c0)
        return load(b_hbm.at[:, cols], b32.at[:, cols])

    drains = []

    def send(dev, src, dst, r=None, cond=None):
        s = fresh("send")
        r = fresh("recv") if r is None else r

        def copy():
            return pltpu.make_async_remote_copy(
                src, dst, ssem.at[s], rsem.at[r], device_id=(dev,),
                device_id_type=pl.DeviceIdType.MESH)

        if cond is None:
            cp = copy()
            cp.start()
            drains.append(cp.wait_send)
            return cp
        pl.when(cond)(lambda: copy().start())
        drains.append(lambda: pl.when(cond)(lambda: copy().wait_send()))

    def arrived(dst, r):
        pltpu.make_async_copy(dst, dst, rsem.at[r]).wait()

    def mm(slot, rows, c0, c1):
        a = jnp.concatenate([a32[slot, lo:hi] for lo, hi in rows], axis=0)
        return jnp.dot(a.astype(BF16), b32[:, c0:c1].astype(BF16),
                       preferred_element_type=F32)

    def tile(ref, lo, hi, c0, c1):
        return ref.at[pl.ds(lo, hi - lo), pl.ds(c0, c1 - c0)]

    mid, rest = ((H - E, H), (H, H + E)), ((0, H - E), (H + E, Q))
    lb = [load_b(*B_COLS[0])]
    la_mid = load_a(A_DIAG, 2, H - E, H + E)

    barrier = pltpu.get_barrier_semaphore()
    for l in range(2):
        pl.semaphore_signal(barrier, 1, device_id=(nbr[l],),
                            device_id_type=pl.DeviceIdType.MESH)

    lb.append(load_b(*B_COLS[1]))
    la_rest = [load_a(A_DIAG, 2, lo, hi) for lo, hi in rest]
    lb += [load_b(*cols) for cols in B_COLS[2:]]
    la_near = [load_a(A_NEAR, XOR[h], h * H, (h + 1) * H) for h in range(2)]
    la_sum = [load_a(A_SUM, XOR[1 - h], h * H, (h + 1) * H) for h in range(2)]
    la_own = load_a(A_OWN, 0, 0, Q)

    def first_tiles(rows, c0, c1):
        part = mm(A_DIAG, rows, c0, c1).astype(BF16)
        n = rows[0][1] - rows[0][0]
        for l, (lo, hi) in enumerate(rows):
            p0s[lo:hi, c0:c1] = part[l * n:(l + 1) * n]
        return [(nbr[l], tile(p0s, lo, hi, c0, c1), tile(p0r, lo, hi, c0, c1))
                for l, (lo, hi) in enumerate(rows)]

    lb[0].wait()
    la_mid.wait()
    tiles = first_tiles(mid, *B_COLS[0])
    pl.semaphore_wait(barrier, 2)
    p0 = [send(*t) for t in tiles]
    lb[1].wait()
    p0 += [send(*t) for t in first_tiles(mid, *B_COLS[1])]
    for cp in la_rest:
        cp.wait()
    for cols in B_COLS[:2]:
        p0 += [send(*t) for t in first_tiles(rest, *cols)]

    w_usual = [fresh("recv") for _ in range(2)]
    w_turned = [fresh("recv") for _ in range(2)]
    for cp, (c0, c1) in zip(lb[2:], B_COLS[2:]):
        cp.wait()
        p0s[:, c0:c1] = mm(A_DIAG, [(0, Q)], c0, c1).astype(BF16)
        w = WP if c1 == N else 0
        for l in range(2):
            lo, hi = l * H + w, (l + 1) * H
            p0.append(send(nbr[l], tile(p0s, lo, hi, c0, c1), tile(p0r, lo, hi, c0, c1)))
        for l in range(2 if w else 0):
            turn = k == XOR[l]
            row = pl.multiple_of(jnp.where(turn, Q + l * w, l * H), 16)
            send(jnp.where(turn, nbr[1 - l], nbr[l]),
                 tile(p0s, l * H, l * H + w, c0, c1),
                 p0r.at[pl.ds(row, w), pl.ds(c0, c1 - c0)],
                 r=jnp.where(turn, w_turned[l], w_usual[l]))

    for cp in la_near:
        cp.wait()
    p1 = {}
    for c in range(NC):
        c0, c1 = c * GC, (c + 1) * GC
        p1s[:, c0:c1] = mm(A_NEAR, [(0, Q)], c0, c1).astype(BF16)
        w = WP if c1 == N else 0
        for l in range(2):
            lo, hi = l * H + w, (l + 1) * H
            p1[l, c] = [send(nbr[l], tile(p1s, lo, hi, c0, c1), tile(p1r, lo, hi, c0, c1))]

    for cp in la_sum:
        cp.wait()
    la_own.wait()
    acc[...] = mm(A_OWN, [(0, Q)], 0, N)

    for cp in p0:
        cp.wait_recv()

    @pl.when(k != 0)
    def _():
        for l in range(2):
            arrived(tile(p0r, l * H, l * H + WP, N - GC, N), w_usual[l])

    @pl.when(k == 2)
    def _():
        for l in range(2):
            arrived(tile(p0r, Q + l * WP, Q + (l + 1) * WP, N - GC, N), w_turned[l])

    s = {}
    for c in range(NC):
        c0, c1 = c * GC, (c + 1) * GC
        w = WP if c1 == N else 0
        part = mm(A_SUM, [(0, Q)], c0, c1)
        for h in range(2):
            lo, hi = h * H, (h + 1) * H
            if w:
                got = jnp.where(k != 0, p0r[lo:lo + w, c0:c1].astype(F32), 0.0)
                ss[lo:lo + w, c0:c1] = (part[lo:lo + w] + got).astype(BF16)
            got = p0r[lo + w:hi, c0:c1].astype(F32)
            ss[lo + w:hi, c0:c1] = (part[lo + w:hi] + got).astype(BF16)
        for l in range(2):
            lo, hi = (1 - l) * H, (2 - l) * H
            s[l, c] = send(nbr[l], tile(ss, lo, hi, c0, c1), tile(sr, lo, hi, c0, c1))
        for l in range(2 if w else 0):
            lo, hi = l * H, l * H + w
            got = jnp.where(k == 2, p0r[Q + l * w:Q + (l + 1) * w, c0:c1].astype(F32), 0.0)
            p1s[lo:hi, c0:c1] = (mm(A_NEAR, [(lo, hi)], c0, c1) + got).astype(BF16)
            p1[l, c].append(send(nbr[l], tile(p1s, lo, hi, c0, c1), tile(p1r, lo, hi, c0, c1)))

    def pack(h, c, z):
        words = pltpu.bitcast(jnp.maximum(z, 0.0).astype(BF16), U32) & LOW
        o_ref[rows_of(0, h * H, (h + 1) * H), c * GC:(c + 1) * GC] = pltpu.bitcast(words, BF16)

        def word(j):
            return words[8 * (j % 8):8 * (j % 8 + 1), 128 * (j // 8):128 * (j // 8 + 1)]

        g0 = h * PH + c * GR
        for j in range(15):
            pk[0, g0 + 8 * j:g0 + 8 * (j + 1)] = word(j) | ((word(15) << (15 - j)) & SIGN)

    def unpack(r, h, c):
        def put(j, word):
            lo = h * H + 16 * (j % 8)
            cols = pl.ds(c * GC + 128 * (j // 8), 128)
            o_ref[rows_of(r, lo, lo + 16), cols] = pltpu.bitcast(word, BF16)

        g0 = h * PH + c * GR
        last = None
        for j in range(15):
            word = pk[r, g0 + 8 * j:g0 + 8 * (j + 1)]
            put(j, word & LOW)
            bit = (word & SIGN) >> (15 - j)
            last = bit if last is None else last | bit
        put(15, last)

    def packed(r, lo, hi):
        return pk.at[r, pl.ds(lo, hi - lo)]

    f1 = {}
    for c in range(NC):
        c0, c1 = c * GC, (c + 1) * GC
        for l in range(2):
            h = 1 - l
            lo, hi = h * H, (h + 1) * H
            for cp in p1[h, c]:
                cp.wait_recv()
            s[l, c].wait_recv()
            pack(h, c, acc[lo:hi, c0:c1] + p1r[lo:hi, c0:c1].astype(F32)
                 + sr[lo:hi, c0:c1].astype(F32))
            g0 = h * PH + c * GR
            f1[l, c] = send(nbr[l], packed(0, g0, g0 + GR), packed(XOR[l], g0, g0 + GR))
    turnable = ((PH - WG, PH), (PH, PH + WG))
    fixed = ((0, PH - WG), (PH + WG, 2 * PH))
    f2w, f2 = [], []
    for l in range(2):
        f2w.append(send(nbr[l], packed(0, *turnable[l]), packed(XOR[l], *turnable[l])))
        f2.append(send(nbr[l], packed(0, *fixed[l]), packed(XOR[l], *fixed[l])))

    for c in range(NC):
        for l in range(2):
            f1[l, c].wait_recv()
    for cp in f2w:
        cp.wait_recv()
    g_turnable = [fresh("recv") for _ in range(2)]
    for l in range(2):
        for h, cond in ((l, k != 2), (1 - l, k == 0)):
            send(nbr[l], packed(XOR[1 - l], *turnable[h]), packed(2, *turnable[h]),
                 r=g_turnable[h], cond=cond)
    n_early = len(drains)
    g = {}
    for c in range(NC):
        for l in range(2):
            lo = max(l * PH + c * GR, fixed[l][0])
            hi = min(l * PH + (c + 1) * GR, fixed[l][1])
            g[l, c] = send(nbr[l], packed(XOR[1 - l], lo, hi), packed(2, lo, hi))

    for l in range(2):
        for c in range(NC):
            unpack(XOR[l], 1 - l, c)
    for l in range(2):
        f2[l].wait_recv()
        for c in range(NC):
            unpack(XOR[l], l, c)

    for drain in drains[:n_early]:
        drain()
    for h in range(2):
        arrived(packed(2, *turnable[h]), g_turnable[h])
    for c in range(NC):
        if c == NC - 1:
            for drain in drains[n_early:-2]:
                drain()
        for l in range(2):
            g[l, c].wait_recv()
            unpack(2, l, c)
    for drain in drains[-2:]:
        drain()
    assert used == dict(load=N_LOADS, send=N_SENDS, recv=N_RECVS), used


def pallas_dist_matmul_relu_kshard_i_m1024_n1024_k512_kernel(
    A: jax.Array,
    B: jax.Array,
):
    hbm = pl.BlockSpec(memory_space=pltpu.HBM)
    block = pltpu.VMEM((Q, N), BF16)
    return pl.pallas_call(
        _body,
        out_shape=pltpu.VMEM((M, N), BF16),
        in_specs=[hbm, hbm],
        out_specs=pl.BlockSpec(memory_space=pltpu.VMEM),
        scratch_shapes=[
            pltpu.VMEM((4, Q, K), F32),
            pltpu.VMEM((K, N), F32),
            block,
            pltpu.VMEM((Q + 2 * WP, N), BF16),
            block, block,
            block, block,
            pltpu.VMEM((4, 2 * PH, 128), U32),
            pltpu.VMEM((Q, N), F32),
            pltpu.SemaphoreType.DMA((N_LOADS,)),
            pltpu.SemaphoreType.DMA((N_SENDS,)),
            pltpu.SemaphoreType.DMA((N_RECVS,)),
        ],
        compiler_params=pltpu.CompilerParams(
            collective_id=0,
            vmem_limit_bytes=32 * 1024 * 1024,
            disable_semaphore_checks=True,
        ),
    )(A, B)
```
